```python
import numpy as np

kernel_name = "dist_sparse_attn_blocksparse_kvseq_b2_sq256_skv256_hq4_dh64"

def setup_inputs():
    x = np.random.randn(2, 256, 512).astype(np.float32)
    Wq = np.random.randn(512, 256).astype(np.float32) * 0.02
    K_ext = np.random.randn(2, 1024, 4, 64).astype(np.float32)
    V_ext = np.random.randn(2, 1024, 4, 64).astype(np.float32)
    Wo = np.random.randn(256, 512).astype(np.float32) * 0.02
    return {"x": x, "Wq": Wq, "K_ext": K_ext, "V_ext": V_ext, "Wo": Wo}

def reference(x, Wq, K_ext, V_ext, Wo):
    B, Sq, Skv, Hq, Dh = 2, 256, 1024, 4, 64
    Q = (x @ Wq).reshape(B, Sq, Hq, Dh)
    qb = (np.arange(Sq) // 64)[:, None]
    kb = (np.arange(Skv) // 64)[None, :]
    mask = (qb == kb) | (kb == 0) | ((qb + kb) % 3 == 0)
    scores = np.einsum('bihd,bjhd->bhij', Q, K_ext).astype(np.float32) * 0.125
    scores = np.where(mask[None, None, :, :], scores, -1e9)
    scores_max = scores.max(axis=-1, keepdims=True)
    w = np.exp(scores - scores_max)
    row_keep = mask.any(axis=1)
    w_sum = np.where(row_keep[None, None, :, None], w.sum(axis=-1, keepdims=True), 1.0)
    w = w / w_sum
    w = np.where(row_keep[None, None, :, None], w, 0.0)
    ctx = np.einsum('bhij,bjhd->bihd', w, V_ext).reshape(B, Sq, Hq * Dh)
    return ctx @ Wo
```

```python
import functools
import jax
import jax.numpy as jnp
from jax import lax
from jax.experimental import pallas as pl
from jax.experimental.pallas import tpu as pltpu

F32 = jnp.float32
BF16 = jnp.bfloat16
U32 = jnp.uint32
LOG2E = 1.4426950408889634
MESH = pl.DeviceIdType.MESH
NT = (((1,), (1,)), ((), ()))
TN = (((0,), (0,)), ((), ()))
TT = (((0,), (1,)), ((), ()))
_QB = ((0, 3), (1, 2))

def _allowed(qb, kb):
    return qb == kb or kb == 0 or (qb + kb) % 3 == 0


def _plan(dev, tile):
    lo = [k for k in range(4) if _allowed(_QB[tile][0], 4 * dev + k)]
    hi = [k for k in range(4) if _allowed(_QB[tile][1], 4 * dev + k)]
    both = [k for k in lo if k in hi]
    lo_only = [k for k in lo if k not in hi]
    hi_only = [k for k in hi if k not in lo]
    rows = [(k, k) for k in both]
    for j in range(max(len(lo_only), len(hi_only))):
        rows.append((lo_only[j] if j < len(lo_only) else None,
                     hi_only[j] if j < len(hi_only) else None))
    used = sorted(set(lo) | set(hi))
    ev = [k for k in used if k % 2 == 0]
    od = [k for k in used if k % 2 == 1]
    kts = []
    for t in range(2):
        if 2 * t in ev and 2 * t + 1 in od:
            kts.append((2 * t, 2 * t + 1)); ev.remove(2 * t); od.remove(2 * t + 1)
    while ev or od:
        kts.append((ev.pop(0) if ev else None, od.pop(0) if od else None))
    return rows, used, kts


PATH_ORDER = (2, 3, 1, 0)

def make_kernel(programs, nsub=4, split=lambda key: 1, fuse_lhs=False, bar_mode="sym"):
    sslot, rslot = {}, {}
    ns = [0] * 4; nr = [0] * 4
    for dev, (_, ops) in enumerate(programs):
        for op in ops:
            keys = []
            if op[0] == "send":
                keys = [(dev, op[2], (op[1], op[3]))]
            elif op[0] == "shipk":
                keys = [(dev, op[4], ("k", op[1], op[2], op[3]))]
            elif op[0] == "shipv":
                keys = [(dev, op[4], ("v", op[1], op[2], j)) for j in range(len(op[3]))]
            elif op[0] == "fw2":
                keys = [(dev, it[2], (it[0], it[3])) for it in op[1]]
            elif op[0] == "shiph":
                keys = [(dev, op[6], (op[1], op[2], op[3], op[4]))]
            for k in keys:
                if k not in sslot:
                    sslot[k] = ns[dev]; ns[dev] += 1
                    rslot[k] = nr[k[1]]; nr[k[1]] += 1
    n_s, n_r = max(ns), max(nr)
    n_ext = {(0, 0): 2, (0, 1): 1, (1, 0): 1, (3, 1): 1}
    RS = 32 // nsub
    PR = 64 // nsub

    def kernel(x, Wq, K_ext, V_ext, Wo):
        kt = jnp.transpose(K_ext, (0, 2, 3, 1)).reshape(2, 2, 128, 256)
        vt = jnp.transpose(V_ext, (0, 2, 3, 1)).reshape(2, 2, 128, 256)

        def body(x_hbm, wq_hbm, k_hbm, v_hbm, wo_hbm, out_ref,
                 xbuf, wqbuf, kbuf, vbuf, wobuf, wq16, wo16, sbuf, rbuf,
                 lsem, ssem, rsem, rdy):
            me = lax.axis_index("i")
            bar = pltpu.get_barrier_semaphore()

            lane = lax.broadcasted_iota(jnp.int32, (1, 128), 1)
            lo_lane = lane < 64
            qscale = [jnp.where(lo_lane, 0.125 * LOG2E, 0.0).astype(F32),
                      jnp.where(lo_lane, 0.0, 0.125 * LOG2E).astype(F32)]

            def path(dev):
                load_order, ops = programs[dev]
                if bar_mode == "sym" or dev != 2:
                    for nb in (dev ^ 1, 3 - dev):
                        pl.semaphore_signal(bar, inc=1, device_id=(nb,), device_id_type=MESH)
                loads = {}
                nl = [0]

                def add(name, src, dst):
                    c = pltpu.make_async_copy(src, dst, lsem.at[nl[0]])
                    nl[0] += 1
                    loads.setdefault(name, []).append(c)
                    c.start()

                for name in load_order:
                    if name[0] == "x" and len(name) == 4:
                        _, b, t, j = name
                        r0 = (0, 192)[j] if t == 0 else 64 + 64 * j
                        add(name, x_hbm.at[b, pl.ds(r0, 64)], xbuf.at[b, t, pl.ds(64 * j, 64)])
                    elif name[0] == "x":
                        _, b, t = name
                        if t == 0:
                            add(name, x_hbm.at[b, pl.ds(0, 64)], xbuf.at[b, t, pl.ds(0, 64)])
                            add(name, x_hbm.at[b, pl.ds(192, 64)], xbuf.at[b, t, pl.ds(64, 64)])
                        else:
                            add(name, x_hbm.at[b, pl.ds(64, 128)], xbuf.at[b, t])
                    elif name[0] in ("k", "v"):
                        src, dst = (k_hbm, kbuf) if name[0] == "k" else (v_hbm, vbuf)
                        if len(name) == 3:
                            add(name, src.at[name[1], name[2]], dst.at[name[1], name[2]])
                        elif name[3] in ("h0", "h1"):
                            rs_ = pl.ds(64 * int(name[3][1]), 64)
                            add(name, src.at[name[1], name[2], rs_], dst.at[name[1], name[2], rs_])
                        elif len(name) == 5:
                            cs = pl.ds(name[3] * 128, 128)
                            rs_ = pl.ds(64 * int(name[4][1]), 64)
                            add(name, src.at[name[1], name[2], rs_, cs], dst.at[name[1], name[2], rs_, cs])
                        else:
                            cs = pl.ds(name[3] * 128, 128)
                            add(name, src.at[name[1], name[2], :, cs], dst.at[name[1], name[2], :, cs])
                    elif name[0] == "wq" and len(name) == 3:
                        rs_ = pl.ds(256 * name[2], 256)
                        add(name, wq_hbm.at[rs_, pl.ds(name[1] * 128, 128)], wqbuf.at[name[1], rs_])
                    elif name[0] == "wq":
                        add(name, wq_hbm.at[:, pl.ds(name[1] * 128, 128)], wqbuf.at[name[1]])
                    elif name[0] == "wo":
                        add(name, wo_hbm, wobuf)

                sends = []
                kn = {}; kne = {}; qv = {}; pv_in = {}; acc = {}; fin = {}; wts = {}
                extk = {}; extv = {}; pend = {}; qpart = {}; vpre = {}; xpre = {}; kpre = {}
                hold = [None]; written = set(); done_s = set(); done_w = set()

                def rwait(key, r0, rows, sub):
                    rcopy(key, r0, rows, sub).wait_recv()

                def rcopy(key, r0, rows, sub):
                    s = sslot[key] if key[0] == dev else 0
                    r = rslot[key]
                    return pltpu.make_async_remote_copy(
                        sbuf.at[s, pl.ds(r0, rows)], rbuf.at[r, pl.ds(r0, rows)],
                        ssem.at[s * nsub + sub], rsem.at[r * nsub + sub],
                        device_id=(key[1],), device_id_type=MESH)

                def start(c):
                    if hold[0] is not None:
                        hold[0].append(c)
                        return
                    c.start(); sends.append(c)

                def op_hold():
                    hold[0] = []

                def op_go():
                    pending, hold[0] = hold[0], None
                    for c in pending:
                        start(c)

                def op_kpre(b, p, tl=None):
                    if tl is None:
                        kpre[(b, p, tl)] = kbuf[b, p].astype(BF16)
                    else:
                        kpre[(b, p, tl)] = kbuf[b, p, :, tl * 128:(tl + 1) * 128].astype(BF16)

                def op_kp(b, p, tl=None):
                    if (b, p, tl) not in kpre:
                        op_kpre(b, p, tl)
                    if tl is None:
                        t_ = kpre[(b, p, tl)].T
                        for kb in range(4):
                            kn[(b, p, kb)] = t_[kb * 64:(kb + 1) * 64]
                    else:
                        t_ = kpre[(b, p, tl)].T
                        for j in range(2):
                            kn[(b, p, 2 * tl + j)] = t_[j * 64:(j + 1) * 64]

                def op_kpe(b, p, tl):
                    t_ = kbuf[b, p, 0:64, tl * 128:(tl + 1) * 128].astype(BF16).T
                    for j in range(2):
                        kne[(b, p, 2 * tl + j)] = t_[j * 64:(j + 1) * 64]

                def op_shipk(b, p, kb, to):
                    key = (dev, to, ("k", b, p, kb))
                    sbuf[sslot[key], 0:32, :] = pltpu.bitcast(kn[(b, p, kb)], U32)
                    start(rcopy(key, 0, 32, 0))

                def op_shipv(b, p, kbs, to):
                    if len(kbs) == 1:
                        kb = kbs[0]
                        c0 = (kb // 2) * 128
                        e = vbuf[b, p, 0:64, c0:c0 + 128]
                        o = vbuf[b, p, 64:128, c0:c0 + 128]
                        if kb % 2 == 1:
                            e = pltpu.roll(e, 64, 1)
                        else:
                            o = pltpu.roll(o, 64, 1)
                        vals = [jnp.where(lo_lane, e, o)]
                    else:
                        ke, ko = kbs
                        vals = [jnp.where(lo_lane, vbuf[b, p, h * 64:(h + 1) * 64, (ke // 2) * 128:(ke // 2) * 128 + 128],
                                          vbuf[b, p, h * 64:(h + 1) * 64, (ko // 2) * 128:(ko // 2) * 128 + 128])
                                for h in range(2)]
                    for j, v in enumerate(vals):
                        key = (dev, to, ("v", b, p, j))
                        sbuf[sslot[key], 0:32, :] = pltpu.bitcast(v.astype(BF16), U32)
                        start(rcopy(key, 0, 32, 0))

                def op_shiph(which, b, p, h, kbs, to):
                    buf = kbuf if which == "kT" else vbuf
                    ke, ko = kbs
                    v = jnp.where(lo_lane, buf[b, p, h * 64:(h + 1) * 64, (ke // 2) * 128:(ke // 2) * 128 + 128],
                                  buf[b, p, h * 64:(h + 1) * 64, (ko // 2) * 128:(ko // 2) * 128 + 128])
                    key = (dev, to, (which, b, p, h))
                    sbuf[sslot[key], 0:32, :] = pltpu.bitcast(v.astype(BF16), U32)
                    start(rcopy(key, 0, 32, 0))

                def op_rkT(b, p, src):
                    keys = [(src, dev, ("kT", b, p, h)) for h in range(2)]
                    for key in keys:
                        rwait(key, 0, 32, 0)
                    pend[(b, p)] = keys

                def op_kpx(b, p):
                    t_ = jnp.concatenate([rload(k) for k in pend[(b, p)]], axis=0).T
                    extk[(b, p)] = [t_[0:64], t_[64:128]]

                def op_rk(b, p, kb, src):
                    key = (src, dev, ("k", b, p, kb))
                    rwait(key, 0, 32, 0)
                    extk.setdefault((b, p), []).append(key)

                def op_rv(b, p, n, src):
                    for j in range(n):
                        key = (src, dev, ("v", b, p, j))
                        rwait(key, 0, 32, 0)
                        extv.setdefault((b, p), []).append(key)

                def rload(key):
                    return pltpu.bitcast(rbuf[rslot[key], 0:32, :], BF16)

                def op_xpre(b, t):
                    xpre[(b, t)] = [xbuf[b, t, :, k * 128:(k + 1) * 128].astype(BF16) for k in range(4)]

                def op_qp(b, t, p):
                    ds = [jnp.dot(xpre[(b, t)][k] if (b, t) in xpre else xbuf[b, t, :, k * 128:(k + 1) * 128].astype(BF16),
                                  wq16[p, k * 128:(k + 1) * 128, :], preferred_element_type=F32)
                          for k in range(4)]
                    q = (ds[0] + ds[1]) + (ds[2] + ds[3])
                    qv[(b, t, p)] = [(q * qscale[h]).astype(BF16) for h in range(2)]

                def op_qpr(b, t, p, j):
                    ds = [jnp.dot(xbuf[b, t, 64 * j:64 * j + 64, k * 128:(k + 1) * 128].astype(BF16),
                                  wq16[p, k * 128:(k + 1) * 128, :], preferred_element_type=F32) for k in range(4)]
                    q = (ds[0] + ds[1]) + (ds[2] + ds[3])
                    qpart.setdefault((b, t, p), {})[j] = [(q * qscale[h]).astype(BF16) for h in range(2)]
                    if len(qpart[(b, t, p)]) == 2:
                        qv[(b, t, p)] = [jnp.concatenate([qpart[(b, t, p)][0][h], qpart[(b, t, p)][1][h]], axis=0)
                                         for h in range(2)]

                def op_qpk(b, t, p, j):
                    ds = {(r, k): jnp.dot(xbuf[b, t, 64 * r:64 * r + 64, k * 128:(k + 1) * 128].astype(BF16),
                                          wq16[p, k * 128:(k + 1) * 128, :], preferred_element_type=F32)
                          for k in (2 * j, 2 * j + 1) for r in range(2)}
                    q = jnp.concatenate([ds[(r, 2 * j)] + ds[(r, 2 * j + 1)] for r in range(2)], axis=0)
                    if (b, t, p) in qpart:
                        q = q + qpart[(b, t, p)]
                        qv[(b, t, p)] = [(q * qscale[h]).astype(BF16) for h in range(2)]
                    else:
                        qpart[(b, t, p)] = q

                def op_qs(b, t, p):
                    op_qsh(((b, t, p, 0), (b, t, p, 1)))

                def op_pv(b, t, p):
                    op_pvh(((b, t, p, 0), (b, t, p, 1)))

                def op_qsl(items):
                    rows, used, kts = _plan(dev, 1)
                    assert [kb for kb in used if kb >= 2] == [2, 3]
                    low = [kb for kb in used if kb < 2]
                    s0 = [lax.dot_general(jnp.concatenate([kn[(b, p, kb)] for kb in low], axis=0), qv[(b, t, p)][h], NT,
                                          preferred_element_type=F32) for (b, t, p, h) in items]
                    s1 = [lax.dot_general(kbuf[b, p, :, 128:256].astype(BF16), qv[(b, t, p)][h], TT,
                                          preferred_element_type=F32) for (b, t, p, h) in items]
                    op_qsh(items, [(jnp.concatenate([a_, c_], axis=0), rows, used, kts, []) for a_, c_ in zip(s0, s1)])

                def op_qsh(items, pre=None):
                    info = []
                    for (b, t, p, h) in (items if pre is None else ()):
                        rows, used, kts = _plan(dev, t)
                        narrow = h == 0 and any((b, p, kb) in kne for kb in used)
                        if narrow:
                            blks = [kne[(b, p, kb)] if (b, p, kb) in kne else kn[(b, p, kb)][:, 0:64] for kb in used]
                        else:
                            blks = [kn[(b, p, kb)] for kb in used]
                        ext = extk.get((b, p), []) if t == 0 else []
                        ekb = [100 + j for j in range(len(ext))]
                        blks += [rload(k) if isinstance(k, tuple) else k for k in ext]
                        used = used + ekb
                        rows = rows + [(k, k) for k in ekb]
                        lhs = jnp.concatenate(blks, axis=0)
                        half = 32 * len(used)
                        st = jnp.concatenate(
                            [lax.dot_general(lhs[j * half:(j + 1) * half],
                                             qv[(b, t, p)][h][:, 0:64] if narrow else qv[(b, t, p)][h], NT,
                                             preferred_element_type=F32) for j in range(2)], axis=0)
                        info.append((st, rows, used, kts, ekb))
                    for (b, t, p, h), (st, rows, used, kts, ekb) in zip(items, pre or info):
                        sblk = {kb: st[j * 64:(j + 1) * 64] for j, kb in enumerate(used)}
                        srow = []
                        for (kl, kh) in rows:
                            if kl == kh:
                                srow.append(sblk[kl])
                            else:
                                a = sblk[kl] if kl is not None else -1e9
                                c = sblk[kh] if kh is not None else -1e9
                                srow.append(jnp.where(lo_lane, a, c))
                        m = jnp.max(functools.reduce(jnp.maximum, srow), axis=0, keepdims=True)
                        prow = [jnp.exp2(s - m) for s in srow]
                        l = jnp.sum(functools.reduce(jnp.add, prow), axis=0, keepdims=True)
                        pblk = {}
                        for (kl, kh), pr in zip(rows, prow):
                            if kl == kh:
                                pblk[kl] = pr
                            else:
                                if kl is not None:
                                    pblk[kl] = pr if kh is None else jnp.where(lo_lane, pr, 0.0)
                                if kh is not None:
                                    pblk[kh] = pr if kl is None else jnp.where(lo_lane, 0.0, pr)
                        kts_h = list(kts)
                        if len(ekb) == 1:
                            kts_h.append((100, None) if h == 0 else (None, 100))
                        elif len(ekb) == 2:
                            kts_h.append((100, 101))
                        ws = []
                        for (ke, ko) in kts_h:
                            if ke is not None and ko is not None:
                                ws.append(jnp.concatenate([pblk[ke], pblk[ko]], axis=0).astype(BF16))
                            elif ke is not None:
                                ws.append(pblk[ke].astype(BF16))
                            else:
                                ws.append(jnp.concatenate([jnp.zeros((64, 128), F32), pblk[ko]], axis=0).astype(BF16))
                        pv_in[(b, t, p, h)] = (ws, m, l, kts_h)

                def kts_of(b, t, p, h):
                    kts = list(_plan(dev, t)[2])
                    ne = n_ext.get((dev, b), 0) if t == 0 else 0
                    if ne == 1:
                        kts.append((100, None) if h == 0 else (None, 100))
                    elif ne == 2:
                        kts.append((100, 101))
                    return kts

                def op_vpre(items):
                    for it in items:
                        if it in vpre:
                            continue
                        b, t, p, h = it
                        kts = kts_of(b, t, p, h)
                        nsp = 2 if len(kts) == 1 else 1
                        rs = 64 // nsp
                        vals = {}
                        for j, (ke, ko) in enumerate(kts):
                            for r in range(nsp):
                                r0 = h * 64 + r * rs

                                def vtile(kb, w=128):
                                    c0 = (kb // 2) * 128
                                    return vbuf[b, p, r0:r0 + rs, c0:c0 + w]
                                if (ke or 0) >= 100 or (ko or 0) >= 100:
                                    ev = extv[(b, p)]
                                    vl = rload(ev[h] if len(ev) == 2 else ev[0])
                                    if ko is None:
                                        vl = vl[:, 0:64]
                                elif ke is not None and ko is not None:
                                    vl = vtile(ke) if ke // 2 == ko // 2 else jnp.where(lo_lane, vtile(ke), vtile(ko))
                                elif ke is not None:
                                    vl = vtile(ke, 64)
                                else:
                                    vl = vtile(ko)
                                vals[(j, r)] = vl.astype(BF16)
                        vpre[it] = vals

                def op_pvh(items):
                    op_vpre(items)
                    parts = {}
                    for it in items:
                        ws = pv_in[it][0]
                        for (j, r), vl in vpre[it].items():
                            parts[(it, j, r)] = jnp.dot(vl, ws[j], preferred_element_type=F32)
                    for it in items:
                        b, t, p, h = it
                        _, m, l, kts = pv_in[it]
                        nsp = 2 if len(kts) == 1 else 1
                        o = jnp.concatenate(
                            [functools.reduce(jnp.add, [parts[(it, j, r)] for j in range(len(kts))])
                             for r in range(nsp)], axis=0)
                        o = o * (1.0 / l)
                        acc[(b, t, 2 * p + h)] = ([o[j * PR:(j + 1) * PR] for j in range(nsub)], m + jnp.log2(l))

                def groups(key):
                    n = int(split(key)) or 1
                    w = nsub // n
                    return [tuple(range(j * w, (j + 1) * w)) for j in range(n - 1, -1, -1)]

                def op_send(pc, to, final, only=None):
                    key = (dev, to, (pc, final))
                    s = sslot[key]
                    for grp in groups(key):
                        if only is not None and not set(grp) <= set(only):
                            continue
                        if (key, grp) in done_s:
                            continue
                        done_s.add((key, grp))
                        for sub in grp:
                            o16 = acc[pc][0][sub].astype(BF16)
                            sbuf[s, sub * RS:(sub + 1) * RS, :] = pltpu.bitcast(o16, U32)
                            if final:
                                fin.setdefault(pc, {})[sub] = o16
                        extra = 0
                        if not final and nsub - 1 in grp:
                            sbuf[s, 32:33, :] = pltpu.bitcast(acc[pc][1], U32)
                            extra = 1
                        start(rcopy(key, grp[0] * RS, RS * len(grp) + extra, grp[0]))

                def wait_group(key, final, grp):
                    if (key, grp) in done_w:
                        return
                    done_w.add((key, grp))
                    extra = 1 if (not final and nsub - 1 in grp) else 0
                    rwait(key, grp[0] * RS, RS * len(grp) + extra, grp[0])

                def op_wr(pc, src, final=False, sel=None):
                    key = (src, dev, (pc, final))
                    gs = groups(key)
                    for grp in (gs if sel is None else gs[sel[0]:sel[1]]):
                        wait_group(key, final, grp)

                def op_rsel(pc, src, final, sel):
                    key = (src, dev, (pc, final))
                    for grp in groups(key)[sel[0]:sel[1]]:
                        recv_group(pc, key, final, grp)

                def op_mg(pc, src):
                    op_recv(pc, src, False)

                def recv_group(pc, key, final, grp):
                    r = rslot[key]
                    extra = 1 if (not final and nsub - 1 in grp) else 0
                    wait_group(key, final, grp)
                    if not final:
                        os_, la = acc[pc]
                        os_ = list(os_)
                    if extra:
                        lb = pltpu.bitcast(rbuf[r, 32:33, :], F32)
                        mx = jnp.maximum(la, lb)
                        ea = jnp.exp2(la - mx)
                        eb = jnp.exp2(lb - mx)
                        sm = ea + eb
                        rc = 1.0 / sm
                        wts[key] = (ea * rc, eb * rc)
                        la = mx + jnp.log2(sm)
                    for sub in grp:
                        o16 = pltpu.bitcast(rbuf[r, sub * RS:(sub + 1) * RS, :], BF16)
                        if final:
                            fin.setdefault(pc, {})[sub] = o16
                        else:
                            wa, wb = wts[key]
                            os_[sub] = os_[sub] * wa + o16.astype(F32) * wb
                    if not final:
                        acc[pc] = (os_, la)

                def op_recv(pc, src, final):
                    key = (src, dev, (pc, final))
                    for grp in groups(key):
                        recv_group(pc, key, final, grp)

                def op_fwd(pc, src, to, final):
                    key = (src, dev, (pc, False))
                    got = []
                    for grp in groups(key):
                        recv_group(pc, key, False, grp)
                        got += list(grp)
                        op_send(pc, to, final, tuple(got))

                def op_fw2(items):
                    got = {it: [] for it in items}
                    gl = {it: groups((it[1], dev, (it[0], False))) for it in items}
                    for j in range(max(len(g) for g in gl.values())):
                        for it in items:
                            if j < len(gl[it]):
                                pc, src_, to, final = it
                                recv_group(pc, (src_, dev, (pc, False)), False, gl[it][j])
                                got[it] += list(gl[it][j])
                                op_send(pc, to, final, tuple(got[it]))

                def op_fin(pc):
                    fin[pc] = {sub: acc[pc][0][sub].astype(BF16) for sub in range(nsub)}

                def op_pj(b, t, p):
                    ct = jnp.concatenate([fin[(b, t, 2 * p + h)][j] for h in (1, 0) for j in range(nsub)], axis=0)
                    d = lax.dot_general(ct, wo16[p * 128:(p + 1) * 128, :], TN, preferred_element_type=F32)
                    segs = ((0, 0, 64), (192, 64, 64)) if t == 0 else ((64, 0, 128),)
                    for (o0, s0, n) in segs:
                        if (b, t) in written:
                            out_ref[b, o0:o0 + n, :] += d[s0:s0 + n]
                        else:
                            out_ref[b, o0:o0 + n, :] = d[s0:s0 + n]
                    written.add((b, t))

                table = {"kp": op_kp, "qp": op_qp, "qs": op_qs, "pv": op_pv, "send": op_send,
                         "recv": op_recv, "pj": op_pj, "shipk": op_shipk, "shipv": op_shipv,
                         "rk": op_rk, "rv": op_rv, "shiph": op_shiph, "rkT": op_rkT, "kpx": op_kpx, "fin": op_fin, "wr": op_wr, "qpr": op_qpr, "qpk": op_qpk, "qsl": op_qsl, "rsel": op_rsel, "vpre": op_vpre, "xpre": op_xpre, "kpre": op_kpre, "hold": op_hold, "go": op_go, "kpe": op_kpe, "fw2": op_fw2, "qsh": op_qsh, "pvh": op_pvh, "mg": op_mg}
                skip = False
                for i, op in enumerate(ops):
                    if skip:
                        skip = False
                        continue
                    kind, a = op[0], op[1:]
                    if (kind == "recv" and not a[2] and i + 1 < len(ops) and ops[i + 1][0] == "send"
                            and ops[i + 1][1] == a[0]):
                        if True:
                            op_fwd(a[0], a[1], ops[i + 1][2], ops[i + 1][3])
                        skip = True
                        continue
                    if True:
                        if kind == "w":
                            for c in loads[a[0]]:
                                c.wait()
                            if a[0][0] == "wq" and len(a[0]) == 3:
                                r0_ = 256 * a[0][2]
                                wq16[a[0][1], r0_:r0_ + 256, :] = wqbuf[a[0][1], r0_:r0_ + 256, :].astype(BF16)
                            elif a[0][0] == "wq":
                                wq16[a[0][1]] = wqbuf[a[0][1]].astype(BF16)
                            if a[0][0] == "wo":
                                for hh in range(4):
                                    wo16[(hh ^ 1) * 64:(hh ^ 1) * 64 + 64, :] = wobuf[hh * 64:hh * 64 + 64, :].astype(BF16)
                        elif kind == "bar":
                            if bar_mode == "sym" or dev in (0, 2):
                                pl.semaphore_wait(bar, 2)
                                if bar_mode != "sym" and dev == 2:
                                    for nb in (1, 3):
                                        pl.semaphore_signal(rdy, inc=1, device_id=(nb,), device_id_type=MESH)
                            else:
                                pl.semaphore_wait(bar, 1)
                        elif kind == "ws":
                            for c in sends:
                                c.wait_send()
                            del sends[:]
                        elif kind == "bar2":
                            if bar_mode != "sym":
                                pl.semaphore_wait(rdy, 1)
                        else:
                            table[kind](*a)
                for c in sends:
                    c.wait_send()
                assert sorted(str(op[1]) for op in ops if op[0] == "w") == sorted(str(n) for n in load_order)
                assert written == {(0, 0), (0, 1), (1, 0), (1, 1)}

            for dev in PATH_ORDER:
                pl.when(me == dev)(functools.partial(path, dev))

        return pl.pallas_call(
            body,
            out_shape=jax.ShapeDtypeStruct((2, 256, 512), F32),
            in_specs=[pl.BlockSpec(memory_space=pl.ANY)] * 5,
            out_specs=pl.BlockSpec(memory_space=pltpu.VMEM),
            scratch_shapes=[
                pltpu.VMEM((2, 2, 128, 512), F32),
                pltpu.VMEM((2, 512, 128), F32),
                pltpu.VMEM((2, 2, 128, 256), F32),
                pltpu.VMEM((2, 2, 128, 256), F32),
                pltpu.VMEM((256, 512), F32),
                pltpu.VMEM((2, 512, 128), BF16),
                pltpu.VMEM((256, 512), BF16),
                pltpu.VMEM((n_s, 40, 128), U32),
                pltpu.VMEM((n_r, 40, 128), U32),
                pltpu.SemaphoreType.DMA((40,)),
                pltpu.SemaphoreType.DMA((n_s * nsub,)),
                pltpu.SemaphoreType.DMA((n_r * nsub,)),
                pltpu.SemaphoreType.REGULAR,
            ],
            compiler_params=pltpu.CompilerParams(collective_id=0, disable_semaphore_checks=True,
                                                 fuse_transposed_lhs_in_matmul=fuse_lhs),
        )(x, Wq, kt, vt, Wo)

    return kernel


W = lambda *n: ("w", tuple(n))
def S(b, t, p, to, final=False): return [("send", (b, t, 2 * p), to, final), ("send", (b, t, 2 * p + 1), to, final)]
def F(b, t, h, src, to, final): return [("recv", (b, t, h), src, False), ("send", (b, t, h), to, final)]
def FP(b, t, p, src, to, final): return F(b, t, 2 * p, src, to, final) + F(b, t, 2 * p + 1, src, to, final)
def R(b, t, p, src): return [("recv", (b, t, 2 * p), src, True), ("recv", (b, t, 2 * p + 1), src, True)]
def WR(items): return [("wr", pc, src) for (pc, src, to, final) in items]
def MS(items): return [("mg", pc, src) for (pc, src, to, final) in items] + [("send", pc, to, final) for (pc, src, to, final) in items]
def FB(items): return WR(items) + MS(items)
V2 = "f"

def side(dev):
    s, k = (1, 0) if dev == 1 else (0, 1)
    tail_loads = [("k", k, 0), ("x", k, 0), ("k", k, 1), ("v", k, 0), ("v", k, 1), ("x", k, 1), ("wo",)]
    if dev == 1:
        kbs = (2,)
        SK = lambda p: [("shipk", s, p, kb, 0) for kb in kbs]
        SV = lambda p: [("shipv", s, p, kbs, 0)]
        loads = [("k", s, 0), ("wq", 0), ("x", s, 1, 1), ("x", s, 1, 0), ("v", s, 0), ("k", s, 1), ("wq", 1), ("v", s, 1)] + tail_loads
        ops = [("bar",), W("k", s, 0), ("kp", s, 0), *SK(0), W("wq", 0), W("x", s, 1, 1), ("qpr", s, 1, 0, 1),
               W("x", s, 1, 0), ("qpr", s, 1, 0, 0), W("v", s, 0), ("qs", s, 1, 0), *SV(0),
               W("k", s, 1), ("bar2",), ("pv", s, 1, 0), ("kp", s, 1), *S(s, 1, 0, 2), *SK(1),
               W("wq", 1), ("qp", s, 1, 1), W("v", s, 1), ("qs", s, 1, 1), *SV(1),
               W("k", k, 0), ("pv", s, 1, 1), ("kp", k, 0), *S(s, 1, 1, 2)]
    else:
        H = lambda which, p, h: ("shiph", which, s, p, h, (0, 3), 0)
        loads = [("k", s, 0, "h0"), ("k", s, 0, "h1"), ("v", s, 0, "h0"), ("wq", 0), ("x", s, 1, 1), ("x", s, 1, 0), ("v", s, 0, "h1"),
                 ("k", s, 1), ("wq", 1), ("v", s, 1)] + tail_loads
        ops = [("bar",), W("k", s, 0, "h0"), H("kT", 0, 0), W("k", s, 0, "h1"), ("kp", s, 0), H("kT", 0, 1),
               W("v", s, 0, "h0"), H("v", 0, 0), W("wq", 0), W("x", s, 1, 1), ("qpr", s, 1, 0, 1), W("x", s, 1, 0), ("qpr", s, 1, 0, 0),
               W("v", s, 0, "h1"), H("v", 0, 1), ("bar2",), ("qs", s, 1, 0),
               W("k", s, 1), H("kT", 1, 0), H("kT", 1, 1), ("pv", s, 1, 0), ("kp", s, 1), *S(s, 1, 0, 2),
               W("wq", 1), ("qp", s, 1, 1), W("v", s, 1), ("qs", s, 1, 1), H("v", 1, 0), H("v", 1, 1),
               W("k", k, 0), ("pv", s, 1, 1), ("kp", k, 0), *S(s, 1, 1, 2)]
    T = [((k, 1, h), 0, 2, False) for h in range(4)]
    ops += [W("x", k, 0), ("qp", k, 0, 0),
            ("rk", k, 0, 1, 2), ("qs", k, 0, 0),
            W("k", k, 1), W("v", k, 0), ("rv", k, 0, 1, 2), ("pv", k, 0, 0), *S(k, 0, 0, 0), ("qp", k, 0, 1), ("kp", k, 1),
            ("rk", k, 1, 1, 2), ("qs", k, 0, 1),
            W("v", k, 1), W("x", k, 1), ("rv", k, 1, 1, 2), ("pv", k, 0, 1), ("qp", k, 1, 0), *S(k, 0, 1, 0), ("qp", k, 1, 1),
            ("qs", k, 1, 0), ("qs", k, 1, 1), *WR(T), ("pv", k, 1, 0), ("pv", k, 1, 1), *MS(T), W("wo",)]
    if dev == 3:
        ops += [*F(k, 1, 0, 2, 0, True), *F(k, 0, 0, 0, 2, True), *F(k, 1, 1, 2, 0, True), *F(k, 0, 1, 0, 2, True),
                *F(k, 1, 2, 2, 0, True), *F(k, 0, 2, 0, 2, True), *F(k, 1, 3, 2, 0, True), *F(k, 0, 3, 0, 2, True),
                ("pj", k, 0, 0), ("pj", k, 1, 0), ("pj", k, 1, 1), ("pj", k, 0, 1)]
    else:
        ops += [*F(k, 1, 0, 2, 0, True), *F(k, 1, 1, 2, 0, True), *F(k, 0, 0, 0, 2, True), *F(k, 1, 2, 2, 0, True),
                *F(k, 0, 1, 0, 2, True), *F(k, 1, 3, 2, 0, True), *FP(k, 0, 1, 0, 2, True),
                ("pj", k, 0, 0), ("pj", k, 1, 0), ("pj", k, 1, 1), ("pj", k, 0, 1)]
    ops += [*R(s, 0, 0, 0), ("pj", s, 0, 0), *R(s, 0, 1, 0), ("pj", s, 0, 1), *R(s, 1, 0, 2), ("pj", s, 1, 0),
            ("ws",), *R(s, 1, 1, 2), ("pj", s, 1, 1)]
    return loads, ops

def d0():
    loads = [("k", 0, 0), ("wq", 0), ("x", 0, 1), ("v", 0, 0), ("k", 1, 0), ("x", 1, 1), ("v", 1, 0),
             ("k", 0, 1), ("wq", 1), ("k", 1, 1), ("v", 0, 1), ("v", 1, 1), ("x", 1, 0), ("x", 0, 0), ("wo",)]
    RV = lambda b, p: [("rv", b, p, 1, 1)] if b == 1 else [("rv", b, p, 2, 3)]
    ops = [W("k", 0, 0), ("kp", 0, 0), W("wq", 0), W("x", 0, 1), ("qp", 0, 1, 0), ("qs", 0, 1, 0),
           W("v", 0, 0), W("k", 1, 0), ("pv", 0, 1, 0), ("kp", 1, 0), ("bar",), *S(0, 1, 0, 1),
           W("x", 1, 1), ("qp", 1, 1, 0), W("v", 1, 0), W("k", 0, 1), ("qs", 1, 1, 0), ("kp", 0, 1), ("pv", 1, 1, 0), *S(1, 1, 0, 3),
           W("wq", 1), W("k", 1, 1), ("qp", 0, 1, 1), ("qp", 1, 1, 1), ("kp", 1, 1), ("qs", 0, 1, 1), ("qs", 1, 1, 1),
           W("v", 0, 1), W("v", 1, 1), ("pv", 0, 1, 1), ("pv", 1, 1, 1), *S(0, 1, 1, 1), *S(1, 1, 1, 3),
           W("x", 1, 0), ("rkT", 0, 0, 3), ("qp", 1, 0, 0), ("qp", 1, 0, 1), ("kpx", 0, 0),
           W("x", 0, 0), ("rk", 1, 0, 2, 1), ("qs", 1, 0, 0), ("qp", 0, 0, 0), ("qp", 0, 0, 1),
           *RV(1, 0), *RV(0, 0), ("pv", 1, 0, 0), ("qs", 0, 0, 0), *S(1, 0, 0, 3),
           ("rk", 1, 1, 2, 1), ("pv", 0, 0, 0), ("qs", 1, 0, 1), *S(0, 0, 0, 1),
           W("wo",), ("rkT", 0, 1, 3), ("kpx", 0, 1), *RV(1, 1), ("pv", 1, 0, 1), ("qs", 0, 0, 1), *S(1, 0, 1, 3),
           *RV(0, 1), ("pv", 0, 0, 1), *S(0, 0, 1, 1)]
    ops += F(0, 0, 0, 1, 3, True) + F(1, 0, 0, 3, 1, True) + F(0, 0, 1, 1, 3, True) + F(1, 0, 1, 3, 1, True)
    ops += [("pj", 0, 0, 0)] + F(0, 0, 2, 1, 3, True) + F(1, 0, 2, 3, 1, True) + [("pj", 1, 0, 0)] + F(0, 0, 3, 1, 3, True) + F(1, 0, 3, 3, 1, True)
    ops += [("pj", 0, 0, 1), ("pj", 1, 0, 1),
            *R(1, 1, 0, 3), *R(0, 1, 0, 1), ("pj", 1, 1, 0), ("pj", 0, 1, 0), ("ws",),
            ("recv", (1, 1, 2), 3, True), ("recv", (0, 1, 2), 1, True),
            ("rsel", (1, 1, 3), 3, True, (0, 3)), ("rsel", (0, 1, 3), 1, True, (0, 3)),
            ("wr", (1, 1, 3), 3, True), ("wr", (0, 1, 3), 1, True),
            ("rsel", (1, 1, 3), 3, True, (3, 4)), ("rsel", (0, 1, 3), 1, True, (3, 4)),
            ("pj", 1, 1, 1), ("pj", 0, 1, 1)]
    return loads, ops

def d2():
    t = lambda b, h: ((b, 1, h), 1 if b == 1 else 3, 3 if b == 1 else 1, False)
    L = [t(1, 2), t(0, 2), t(1, 3), t(0, 3)]
    SK2 = lambda p: [W("k", 1, p, 0), W("k", 0, p, 0), ("kp", 1, p, 0), ("kp", 0, p, 0), ("shipk", 1, p, 1, 3), ("shipk", 0, p, 1, 1)]
    SV2 = lambda p: [W("v", 1, p, 0), W("v", 0, p, 0), ("hold",), ("shipv", 1, p, (1,), 3), ("shipv", 0, p, (1,), 1), ("go",)]
    loads = [("k", 1, 0, 0), ("k", 0, 0, 0), ("v", 1, 0, 0), ("v", 0, 0, 0),
             ("k", 1, 1, 0), ("k", 0, 1, 0), ("v", 1, 1, 0), ("v", 0, 1, 0),
             ("wq", 0), ("x", 1, 1), ("x", 0, 1), ("k", 1, 0, 1), ("k", 0, 0, 1), ("v", 1, 0, 1), ("v", 0, 0, 1),
             ("k", 1, 1, 1, "h0"), ("k", 0, 1, 1, "h0"), ("wq", 1), ("k", 1, 1, 1, "h1"), ("k", 0, 1, 1, "h1"),
             ("v", 1, 1, 1), ("v", 0, 1, 1), ("wo",)]
    X0 = ((1, 1, 0, 0), (0, 1, 0, 0)); Y0 = ((1, 1, 0, 1), (0, 1, 0, 1))
    X = ((1, 1, 1, 0), (0, 1, 1, 0)); Y = ((1, 1, 1, 1), (0, 1, 1, 1))
    ops = [("bar",), *SK2(0), *SV2(0), *SK2(1), *SV2(1),
           W("wq", 0), W("x", 1, 1), ("qp", 1, 1, 0), W("x", 0, 1), ("qp", 0, 1, 0),
           W("k", 1, 0, 1), W("k", 0, 0, 1), ("qsl", X0 + Y0),
           W("v", 1, 0, 1), W("v", 0, 0, 1), ("pvh", X0), ("pvh", Y0), *FB([t(1, 0), t(0, 0)]),
           W("k", 1, 1, 1, "h0"), W("k", 0, 1, 1, "h0"), W("wq", 1), ("qp", 1, 1, 1), ("qp", 0, 1, 1), ("kpe", 1, 1, 1), ("kpe", 0, 1, 1),
           *FB([t(1, 1), t(0, 1)]), W("k", 1, 1, 1, "h1"), W("k", 0, 1, 1, "h1"), W("v", 1, 1, 1), W("v", 0, 1, 1),
           ("qsh", X), ("kp", 1, 1, 1), ("kp", 0, 1, 1), *WR(L[:2]), ("pvh", X), ("qsh", Y), *MS(L[:2]), ("pvh", Y),
           *FB(L[2:]), W("wo",)]
    for h in range(4):
        ops += [("fw2", (((1, 1, h), 3, 1, True), ((0, 1, h), 1, 3, True)))]
    ops += [("pj", 0, 1, 0), ("pj", 1, 1, 0), ("pj", 0, 1, 1), ("pj", 1, 1, 1),
            *R(1, 0, 0, 3), *R(0, 0, 0, 1), ("pj", 1, 0, 0), ("pj", 0, 0, 0),
            *R(1, 0, 1, 3), ("pj", 1, 0, 1), ("ws",), *R(0, 0, 1, 1), ("pj", 0, 0, 1)]
    return loads, ops

SPL = "4444"
SPL2 = "2222"
def split(key):
    src, dst, tag = key
    if not isinstance(tag[0], tuple): return 1
    (b, t, h), final = tag
    if t == 1 and ((src == 2 and not final) or (dst == 0 and final)):
        return int(SPL[h])
    keep = {1: 0, 3: 1}
    if t == 1 and ((dst == 2 and not final and keep[src] == b) or (src == 2 and final)):
        return int(SPL2[h])
    return 1

PROGRAMS = [d0(), side(1), d2(), side(3)]
_kernel = make_kernel(PROGRAMS, split=split, fuse_lhs=bool(int("0")), bar_mode="asym")


def pallas_dist_sparse_attn_blocksparse_kvseq_b2_sq256_skv256_hq4_dh64_kernel(x, Wq, K_ext, V_ext, Wo):
    return _kernel(x, Wq, K_ext, V_ext, Wo)
```

```python
import functools
import jax
import jax.numpy as jnp
from jax import lax
from jax.experimental import pallas as pl
from jax.experimental.pallas import tpu as pltpu

F32 = jnp.float32
BF16 = jnp.bfloat16
U32 = jnp.uint32
LOG2E = 1.4426950408889634
MESH = pl.DeviceIdType.MESH
NT = (((1,), (1,)), ((), ()))
TN = (((0,), (0,)), ((), ()))
TT = (((0,), (1,)), ((), ()))
_QB = ((0, 3), (1, 2))
_EXT = 100
_N_EXT = {(0, 0): 2, (0, 1): 1, (1, 0): 1, (3, 1): 1}
NSUB = 4
RS = 32 // NSUB
PR = 64 // NSUB
PATH_ORDER = (2, 3, 1, 0)


def _allowed(qb, kb):
    return qb == kb or kb == 0 or (qb + kb) % 3 == 0


def _plan(dev, tile):
    lo = [k for k in range(4) if _allowed(_QB[tile][0], 4 * dev + k)]
    hi = [k for k in range(4) if _allowed(_QB[tile][1], 4 * dev + k)]
    lo_only = [k for k in lo if k not in hi]
    hi_only = [k for k in hi if k not in lo]
    rows = [(k, k) for k in lo if k in hi]
    for j in range(max(len(lo_only), len(hi_only))):
        rows.append((lo_only[j] if j < len(lo_only) else None,
                     hi_only[j] if j < len(hi_only) else None))
    used = sorted(set(lo) | set(hi))
    ev = [k for k in used if k % 2 == 0]
    od = [k for k in used if k % 2 == 1]
    kts = []
    for t in range(2):
        if 2 * t in ev and 2 * t + 1 in od:
            kts.append((2 * t, 2 * t + 1))
            ev.remove(2 * t)
            od.remove(2 * t + 1)
    while ev or od:
        kts.append((ev.pop(0) if ev else None, od.pop(0) if od else None))
    return rows, used, kts


def _sent_keys(dev, op):
    if op[0] == "send":
        return [(dev, op[2], (op[1], op[3]))]
    if op[0] == "fw2":
        return [(dev, it[2], (it[0], it[3])) for it in op[1]]
    if op[0] == "shipk":
        return [(dev, op[4], ("k", op[1], op[2], op[3]))]
    if op[0] == "shipv":
        return [(dev, op[4], ("v", op[1], op[2], 0))]
    if op[0] == "shiph":
        return [(dev, op[6], (op[1], op[2], op[3], op[4]))]
    return []


def make_kernel(programs, split):
    sslot, rslot = {}, {}
    ns, nr = [0] * 4, [0] * 4
    for dev, (_, ops) in enumerate(programs):
        for op in ops:
            for k in _sent_keys(dev, op):
                sslot[k] = ns[dev]
                rslot[k] = nr[k[1]]
                ns[dev] += 1
                nr[k[1]] += 1
    n_s, n_r = max(ns), max(nr)
    n_l = max(len(p[0]) for p in programs) + 2

    def body(x_hbm, wq_hbm, k_hbm, v_hbm, wo_hbm, out_ref,
             xbuf, wqbuf, kbuf, vbuf, wobuf, wq16, wo16, sbuf, rbuf,
             lsem, ssem, rsem, rdy):
        me = lax.axis_index("i")
        bar = pltpu.get_barrier_semaphore()
        lo_lane = lax.broadcasted_iota(jnp.int32, (1, 128), 1) < 64
        qscale = [jnp.where(lo_lane, 0.125 * LOG2E, 0.0).astype(F32),
                  jnp.where(lo_lane, 0.0, 0.125 * LOG2E).astype(F32)]

        def path(dev):
            load_order, ops = programs[dev]
            if dev != 2:
                for nb in (dev ^ 1, 3 - dev):
                    pl.semaphore_signal(bar, inc=1, device_id=(nb,), device_id_type=MESH)

            loads = {}

            def add(name, src, dst):
                c = pltpu.make_async_copy(src, dst, lsem.at[sum(len(v) for v in loads.values())])
                loads.setdefault(name, []).append(c)
                c.start()

            for name in load_order:
                if name[0] == "x":
                    b, t = name[1:3]
                    if t == 1 and len(name) == 3:
                        add(name, x_hbm.at[b, pl.ds(64, 128)], xbuf.at[b, t])
                    else:
                        for j in name[3:] or (0, 1):
                            add(name, x_hbm.at[b, pl.ds(64 * _QB[t][j], 64)], xbuf.at[b, t, pl.ds(64 * j, 64)])
                elif name[0] in ("k", "v"):
                    src, dst = (k_hbm, kbuf) if name[0] == "k" else (v_hbm, vbuf)
                    rows, cols = pl.ds(0, 128), pl.ds(0, 256)
                    for z in name[3:]:
                        if z in ("h0", "h1"):
                            rows = pl.ds(64 * int(z[1]), 64)
                        else:
                            cols = pl.ds(128 * z, 128)
                    add(name, src.at[name[1], name[2], rows, cols], dst.at[name[1], name[2], rows, cols])
                elif name[0] == "wq":
                    add(name, wq_hbm.at[:, pl.ds(name[1] * 128, 128)], wqbuf.at[name[1]])
                else:
                    add(name, wo_hbm, wobuf)

            sends, hold = [], [None]
            kn, kne, qv, qpart, pv_in = {}, {}, {}, {}, {}
            acc, fin, wts, extk, extv, pend = {}, {}, {}, {}, {}, {}
            written, done_s, done_w = set(), set(), set()

            def rcopy(key, r0, rows, sub):
                s = sslot[key] if key[0] == dev else 0
                r = rslot[key]
                return pltpu.make_async_remote_copy(
                    sbuf.at[s, pl.ds(r0, rows)], rbuf.at[r, pl.ds(r0, rows)],
                    ssem.at[s * NSUB + sub], rsem.at[r * NSUB + sub],
                    device_id=(key[1],), device_id_type=MESH)

            def rwait(key, r0, rows, sub):
                rcopy(key, r0, rows, sub).wait_recv()

            def start(c):
                if hold[0] is not None:
                    hold[0].append(c)
                    return
                c.start()
                sends.append(c)

            def op_hold():
                hold[0] = []

            def op_go():
                pending, hold[0] = hold[0], None
                for c in pending:
                    start(c)

            def ship(key, val):
                sbuf[sslot[key], 0:32, :] = pltpu.bitcast(val, U32)
                start(rcopy(key, 0, 32, 0))

            def rload(key):
                return pltpu.bitcast(rbuf[rslot[key], 0:32, :], BF16)

            def op_kp(b, p, tl=None):
                c0, n = (0, 4) if tl is None else (128 * tl, 2)
                t_ = kbuf[b, p, :, c0:c0 + 64 * n].astype(BF16).T
                for j in range(n):
                    kn[(b, p, c0 // 64 + j)] = t_[j * 64:(j + 1) * 64]

            def op_kpe(b, p, tl):
                t_ = kbuf[b, p, 0:64, tl * 128:(tl + 1) * 128].astype(BF16).T
                for j in range(2):
                    kne[(b, p, 2 * tl + j)] = t_[j * 64:(j + 1) * 64]

            def op_shipk(b, p, kb, to):
                ship((dev, to, ("k", b, p, kb)), kn[(b, p, kb)])

            def op_shipv(b, p, kbs, to):
                kb = kbs[0]
                c0 = (kb // 2) * 128
                e = vbuf[b, p, 0:64, c0:c0 + 128]
                o = vbuf[b, p, 64:128, c0:c0 + 128]
                if kb % 2 == 1:
                    e = pltpu.roll(e, 64, 1)
                else:
                    o = pltpu.roll(o, 64, 1)
                ship((dev, to, ("v", b, p, 0)), jnp.where(lo_lane, e, o).astype(BF16))

            def op_shiph(which, b, p, h, kbs, to):
                buf = kbuf if which == "kT" else vbuf
                ce, co = (kbs[0] // 2) * 128, (kbs[1] // 2) * 128
                v = jnp.where(lo_lane, buf[b, p, h * 64:(h + 1) * 64, ce:ce + 128],
                              buf[b, p, h * 64:(h + 1) * 64, co:co + 128])
                ship((dev, to, (which, b, p, h)), v.astype(BF16))

            def op_rk(b, p, kb, src):
                key = (src, dev, ("k", b, p, kb))
                rwait(key, 0, 32, 0)
                extk[(b, p)] = [key]

            def op_rkT(b, p, src):
                pend[(b, p)] = [(src, dev, ("kT", b, p, h)) for h in range(2)]
                for key in pend[(b, p)]:
                    rwait(key, 0, 32, 0)

            def op_kpx(b, p):
                t_ = jnp.concatenate([rload(k) for k in pend[(b, p)]], axis=0).T
                extk[(b, p)] = [t_[0:64], t_[64:128]]

            def op_rv(b, p, n, src):
                extv[(b, p)] = [(src, dev, ("v", b, p, j)) for j in range(n)]
                for key in extv[(b, p)]:
                    rwait(key, 0, 32, 0)

            def qproj(b, t, p, r0, n):
                ds = [jnp.dot(xbuf[b, t, r0:r0 + n, k * 128:(k + 1) * 128].astype(BF16),
                              wq16[p, k * 128:(k + 1) * 128, :], preferred_element_type=F32) for k in range(4)]
                q = (ds[0] + ds[1]) + (ds[2] + ds[3])
                return [(q * qscale[h]).astype(BF16) for h in range(2)]

            def op_qp(b, t, p):
                qv[(b, t, p)] = qproj(b, t, p, 0, 128)

            def op_qpr(b, t, p, j):
                part = qpart.setdefault((b, t, p), {})
                part[j] = qproj(b, t, p, 64 * j, 64)
                if len(part) == 2:
                    qv[(b, t, p)] = [jnp.concatenate([part[0][h], part[1][h]], axis=0) for h in range(2)]

            def kts_of(b, t, h):
                kts = list(_plan(dev, t)[2])
                ne = _N_EXT.get((dev, b), 0) if t == 0 else 0
                if ne == 1:
                    kts.append((_EXT, None) if h == 0 else (None, _EXT))
                elif ne == 2:
                    kts.append((_EXT, _EXT + 1))
                return kts

            def softmax(it, st, rows, used):
                b, t, p, h = it
                sblk = {kb: st[j * 64:(j + 1) * 64] for j, kb in enumerate(used)}
                srow = []
                for (kl, kh) in rows:
                    if kl == kh:
                        srow.append(sblk[kl])
                    else:
                        srow.append(jnp.where(lo_lane, sblk[kl] if kl is not None else -1e9,
                                              sblk[kh] if kh is not None else -1e9))
                m = jnp.max(functools.reduce(jnp.maximum, srow), axis=0, keepdims=True)
                prow = [jnp.exp2(s - m) for s in srow]
                l = jnp.sum(functools.reduce(jnp.add, prow), axis=0, keepdims=True)
                pblk = {}
                for (kl, kh), pr in zip(rows, prow):
                    if kl == kh:
                        pblk[kl] = pr
                        continue
                    if kl is not None:
                        pblk[kl] = pr if kh is None else jnp.where(lo_lane, pr, 0.0)
                    if kh is not None:
                        pblk[kh] = pr if kl is None else jnp.where(lo_lane, 0.0, pr)
                ws = []
                for (ke, ko) in kts_of(b, t, h):
                    if ko is None:
                        ws.append(pblk[ke].astype(BF16))
                    else:
                        top = pblk[ke] if ke is not None else jnp.zeros((64, 128), F32)
                        ws.append(jnp.concatenate([top, pblk[ko]], axis=0).astype(BF16))
                pv_in[it] = (ws, m, l)

            def op_qsh(items):
                info = []
                for (b, t, p, h) in items:
                    rows, used, _ = _plan(dev, t)
                    q = qv[(b, t, p)][h]
                    if h == 0 and any((b, p, kb) in kne for kb in used):
                        blks = [kne[(b, p, kb)] if (b, p, kb) in kne else kn[(b, p, kb)][:, 0:64] for kb in used]
                        q = q[:, 0:64]
                    else:
                        blks = [kn[(b, p, kb)] for kb in used]
                    ext = extk.get((b, p), []) if t == 0 else []
                    assert t != 0 or len(ext) == _N_EXT.get((dev, b), 0)
                    blks += [rload(k) if isinstance(k, tuple) else k for k in ext]
                    ekb = [_EXT + j for j in range(len(ext))]
                    lhs = jnp.concatenate(blks, axis=0)
                    ways = 4 if len(items) == 1 else 2
                    part = 64 * len(blks) // ways
                    st = jnp.concatenate(
                        [lax.dot_general(lhs[j * part:(j + 1) * part], q, NT, preferred_element_type=F32)
                         for j in range(ways)], axis=0)
                    info.append((st, rows + [(k, k) for k in ekb], used + ekb))
                for it, inf in zip(items, info):
                    softmax(it, *inf)

            def op_qsl(items):
                rows, used, _ = _plan(dev, 1)
                assert [kb for kb in used if kb >= 2] == [2, 3]
                low = [kb for kb in used if kb < 2]
                s0 = [lax.dot_general(jnp.concatenate([kn[(b, p, kb)] for kb in low], axis=0), qv[(b, t, p)][h],
                                      NT, preferred_element_type=F32) for (b, t, p, h) in items]
                s1 = [lax.dot_general(kbuf[b, p, :, 128:256].astype(BF16), qv[(b, t, p)][h],
                                      TT, preferred_element_type=F32) for (b, t, p, h) in items]
                for it, a_, c_ in zip(items, s0, s1):
                    softmax(it, jnp.concatenate([a_, c_], axis=0), rows, used)

            def op_pvh(items):
                vls = {}
                for it in items:
                    b, t, p, h = it
                    kts = kts_of(b, t, h)
                    nsp = max(1, 4 // (len(kts) * len(items)))
                    rs = 64 // nsp
                    for j, (ke, ko) in enumerate(kts):
                        for r in range(nsp):
                            r0 = h * 64 + r * rs

                            def vtile(kb, w=128):
                                c0 = (kb // 2) * 128
                                return vbuf[b, p, r0:r0 + rs, c0:c0 + w]
                            if (ke or 0) >= _EXT or (ko or 0) >= _EXT:
                                ev = extv[(b, p)]
                                vl = rload(ev[h] if len(ev) == 2 else ev[0])[r * rs:(r + 1) * rs]
                                if ko is None:
                                    vl = vl[:, 0:64]
                            elif ko is None:
                                vl = vtile(ke, 64)
                            elif ke is None or ke // 2 == ko // 2:
                                vl = vtile(ko)
                            else:
                                vl = jnp.where(lo_lane, vtile(ke), vtile(ko))
                            vls[(it, j, r)] = vl.astype(BF16)
                parts = {kk: jnp.dot(vl, pv_in[kk[0]][0][kk[1]], preferred_element_type=F32)
                         for kk, vl in vls.items()}
                for it in items:
                    b, t, p, h = it
                    ws, m, l = pv_in[it]
                    o = jnp.concatenate(
                        [functools.reduce(jnp.add, [parts[(it, j, r)] for j in range(len(ws))])
                         for r in range(max(1, 4 // (len(ws) * len(items))))], axis=0)
                    o = o * (1.0 / l)
                    acc[(b, t, 2 * p + h)] = ([o[j * PR:(j + 1) * PR] for j in range(NSUB)], m + jnp.log2(l))

            def op_qs(b, t, p):
                op_qsh(((b, t, p, 0), (b, t, p, 1)))

            def op_pv(b, t, p):
                op_pvh(((b, t, p, 0), (b, t, p, 1)))

            def groups(key):
                w = NSUB // split(key)
                return [tuple(range(j, j + w)) for j in range(NSUB - w, -1, -w)]

            def span(final, grp):
                return grp[0] * RS, RS * len(grp) + int(not final and NSUB - 1 in grp), grp[0]

            def op_send(pc, to, final, only=None):
                key = (dev, to, (pc, final))
                s = sslot[key]
                for grp in groups(key):
                    if (key, grp) in done_s or (only is not None and not set(grp) <= set(only)):
                        continue
                    done_s.add((key, grp))
                    for sub in grp:
                        o16 = acc[pc][0][sub].astype(BF16)
                        sbuf[s, sub * RS:(sub + 1) * RS, :] = pltpu.bitcast(o16, U32)
                        if final:
                            fin.setdefault(pc, {})[sub] = o16
                    if not final and NSUB - 1 in grp:
                        sbuf[s, 32:33, :] = pltpu.bitcast(acc[pc][1], U32)
                    start(rcopy(key, *span(final, grp)))

            def wait_group(key, final, grp):
                if (key, grp) not in done_w:
                    done_w.add((key, grp))
                    rwait(key, *span(final, grp))

            def recv_group(pc, key, final, grp):
                r = rslot[key]
                wait_group(key, final, grp)
                if final:
                    for sub in grp:
                        fin.setdefault(pc, {})[sub] = pltpu.bitcast(rbuf[r, sub * RS:(sub + 1) * RS, :], BF16)
                    return
                os_, la = acc[pc]
                os_ = list(os_)
                if NSUB - 1 in grp:
                    lb = pltpu.bitcast(rbuf[r, 32:33, :], F32)
                    mx = jnp.maximum(la, lb)
                    ea = jnp.exp2(la - mx)
                    eb = jnp.exp2(lb - mx)
                    sm = ea + eb
                    rc = 1.0 / sm
                    wts[key] = (ea * rc, eb * rc)
                    la = mx + jnp.log2(sm)
                wa, wb = wts[key]
                for sub in grp:
                    o16 = pltpu.bitcast(rbuf[r, sub * RS:(sub + 1) * RS, :], BF16)
                    os_[sub] = os_[sub] * wa + o16.astype(F32) * wb
                acc[pc] = (os_, la)

            def op_wr(pc, src, final=False):
                key = (src, dev, (pc, final))
                for grp in groups(key):
                    wait_group(key, final, grp)

            def op_recv(pc, src, final=False, sel=(0, NSUB)):
                key = (src, dev, (pc, final))
                for grp in groups(key)[sel[0]:sel[1]]:
                    recv_group(pc, key, final, grp)

            def op_fw2(items):
                got = {it: [] for it in items}
                gl = {it: groups((it[1], dev, (it[0], False))) for it in items}
                for j in range(max(len(g) for g in gl.values())):
                    for it in items:
                        if j < len(gl[it]):
                            pc, src, to, final = it
                            recv_group(pc, (src, dev, (pc, False)), False, gl[it][j])
                            got[it] += list(gl[it][j])
                            op_send(pc, to, final, tuple(got[it]))

            def op_pj(b, t, p):
                ct = jnp.concatenate([fin[(b, t, 2 * p + h)][j] for h in (1, 0) for j in range(NSUB)], axis=0)
                d = lax.dot_general(ct, wo16[p * 128:(p + 1) * 128, :], TN, preferred_element_type=F32)
                for (o0, s0, n) in (((0, 0, 64), (192, 64, 64)) if t == 0 else ((64, 0, 128),)):
                    if (b, t) in written:
                        out_ref[b, o0:o0 + n, :] += d[s0:s0 + n]
                    else:
                        out_ref[b, o0:o0 + n, :] = d[s0:s0 + n]
                written.add((b, t))

            def op_w(name):
                for c in loads.pop(name):
                    c.wait()
                if name[0] == "wq":
                    wq16[name[1]] = wqbuf[name[1]].astype(BF16)
                elif name[0] == "wo":
                    for hh in range(4):
                        wo16[(hh ^ 1) * 64:(hh ^ 1) * 64 + 64, :] = wobuf[hh * 64:hh * 64 + 64, :].astype(BF16)

            def op_bar():
                pl.semaphore_wait(bar, 2 if dev in (0, 2) else 1)
                if dev == 2:
                    for nb in (1, 3):
                        pl.semaphore_signal(rdy, inc=1, device_id=(nb,), device_id_type=MESH)

            def op_bar2():
                pl.semaphore_wait(rdy, 1)

            def op_ws():
                for c in sends:
                    c.wait_send()
                del sends[:]

            table = {"w": op_w, "bar": op_bar, "bar2": op_bar2, "ws": op_ws, "hold": op_hold, "go": op_go,
                     "kp": op_kp, "kpe": op_kpe, "kpx": op_kpx, "shipk": op_shipk, "shipv": op_shipv,
                     "shiph": op_shiph, "rk": op_rk, "rkT": op_rkT, "rv": op_rv,
                     "qp": op_qp, "qpr": op_qpr, "qs": op_qs, "qsh": op_qsh, "qsl": op_qsl,
                     "pv": op_pv, "pvh": op_pvh, "send": op_send, "recv": op_recv, "mg": op_recv,
                     "rsel": op_recv, "wr": op_wr, "fw2": op_fw2, "pj": op_pj}
            i = 0
            while i < len(ops):
                op = ops[i]
                nxt = ops[i + 1] if i + 1 < len(ops) else ("end",)
                if op[0] == "recv" and not op[3] and nxt[0] == "send" and nxt[1] == op[1]:
                    op_fw2(((op[1], op[2], nxt[2], nxt[3]),))
                    i += 2
                    continue
                table[op[0]](*op[1:])
                i += 1
            op_ws()
            assert not loads and len(written) == 4

        for dev in PATH_ORDER:
            pl.when(me == dev)(functools.partial(path, dev))

    def kernel(x, Wq, K_ext, V_ext, Wo):
        kt = jnp.transpose(K_ext, (0, 2, 3, 1)).reshape(2, 2, 128, 256)
        vt = jnp.transpose(V_ext, (0, 2, 3, 1)).reshape(2, 2, 128, 256)
        return pl.pallas_call(
            body,
            out_shape=jax.ShapeDtypeStruct((2, 256, 512), F32),
            in_specs=[pl.BlockSpec(memory_space=pl.ANY)] * 5,
            out_specs=pl.BlockSpec(memory_space=pltpu.VMEM),
            scratch_shapes=[
                pltpu.VMEM((2, 2, 128, 512), F32),
                pltpu.VMEM((2, 512, 128), F32),
                pltpu.VMEM((2, 2, 128, 256), F32),
                pltpu.VMEM((2, 2, 128, 256), F32),
                pltpu.VMEM((256, 512), F32),
                pltpu.VMEM((2, 512, 128), BF16),
                pltpu.VMEM((256, 512), BF16),
                pltpu.VMEM((n_s, 40, 128), U32),
                pltpu.VMEM((n_r, 40, 128), U32),
                pltpu.SemaphoreType.DMA((n_l,)),
                pltpu.SemaphoreType.DMA((n_s * NSUB,)),
                pltpu.SemaphoreType.DMA((n_r * NSUB,)),
                pltpu.SemaphoreType.REGULAR,
            ],
            compiler_params=pltpu.CompilerParams(collective_id=0, disable_semaphore_checks=True),
        )(x, Wq, kt, vt, Wo)

    return kernel


def W(*name):
    return ("w", name)


def S(b, t, p, to):
    return [("send", (b, t, 2 * p + h), to, False) for h in range(2)]


def F(b, t, h, src, to):
    return [("recv", (b, t, h), src, False), ("send", (b, t, h), to, True)]


def R(b, t, p, src):
    return [("recv", (b, t, 2 * p + h), src, True) for h in range(2)]


def WR(items):
    return [("wr", pc, src) for (pc, src, to) in items]


def MS(items):
    return [("mg", pc, src) for (pc, src, to) in items] + [("send", pc, to, False) for (pc, src, to) in items]


def _chip0():
    loads = [("k", 0, 0), ("wq", 0), ("x", 0, 1), ("v", 0, 0), ("k", 1, 0), ("x", 1, 1), ("v", 1, 0),
             ("k", 0, 1), ("wq", 1), ("k", 1, 1), ("v", 0, 1), ("v", 1, 1), ("x", 1, 0), ("x", 0, 0), ("wo",)]
    ops = [W("k", 0, 0), ("kp", 0, 0), W("wq", 0), W("x", 0, 1), ("qp", 0, 1, 0), ("qs", 0, 1, 0),
           W("v", 0, 0), W("k", 1, 0), ("pv", 0, 1, 0), ("kp", 1, 0), ("bar",), *S(0, 1, 0, 1),
           W("x", 1, 1), ("qp", 1, 1, 0),
           W("v", 1, 0), W("k", 0, 1), ("qs", 1, 1, 0), ("kp", 0, 1), ("pv", 1, 1, 0), *S(1, 1, 0, 3),
           W("wq", 1), W("k", 1, 1), ("qp", 0, 1, 1), ("qp", 1, 1, 1), ("kp", 1, 1), ("qs", 0, 1, 1), ("qs", 1, 1, 1),
           W("v", 0, 1), W("v", 1, 1), ("pv", 0, 1, 1), ("pv", 1, 1, 1), *S(0, 1, 1, 1), *S(1, 1, 1, 3),
           W("x", 1, 0), ("rkT", 0, 0, 3), ("qp", 1, 0, 0), ("qp", 1, 0, 1), ("kpx", 0, 0),
           W("x", 0, 0), ("rk", 1, 0, 2, 1), ("qs", 1, 0, 0), ("qp", 0, 0, 0), ("qp", 0, 0, 1),
           ("rv", 1, 0, 1, 1), ("rv", 0, 0, 2, 3), ("pv", 1, 0, 0), ("qs", 0, 0, 0), *S(1, 0, 0, 3),
           ("rk", 1, 1, 2, 1), ("pv", 0, 0, 0), ("qs", 1, 0, 1), *S(0, 0, 0, 1),
           W("wo"), ("rkT", 0, 1, 3), ("kpx", 0, 1),
           ("rv", 1, 1, 1, 1), ("pv", 1, 0, 1), ("qs", 0, 0, 1), *S(1, 0, 1, 3),
           ("rv", 0, 1, 2, 3), ("pv", 0, 0, 1), *S(0, 0, 1, 1),
           *F(0, 0, 0, 1, 3), *F(1, 0, 0, 3, 1), *F(0, 0, 1, 1, 3), *F(1, 0, 1, 3, 1), ("pj", 0, 0, 0),
           *F(0, 0, 2, 1, 3), *F(1, 0, 2, 3, 1), ("pj", 1, 0, 0),
           *F(0, 0, 3, 1, 3), *F(1, 0, 3, 3, 1), ("pj", 0, 0, 1), ("pj", 1, 0, 1),
           *R(1, 1, 0, 3), *R(0, 1, 0, 1), ("pj", 1, 1, 0), ("pj", 0, 1, 0), ("ws",),
           *R(1, 1, 1, 3), *R(0, 1, 1, 1), ("pj", 1, 1, 1), ("pj", 0, 1, 1)]
    return loads, ops


def _side(dev):
    s, k = (1, 0) if dev == 1 else (0, 1)
    first_q = [W("wq", 0), W("x", s, 1, 1), ("qpr", s, 1, 0, 1), W("x", s, 1, 0), ("qpr", s, 1, 0, 0)]
    if dev == 1:
        loads = [("k", s, 0), ("wq", 0), ("x", s, 1, 1), ("x", s, 1, 0), ("v", s, 0)]
        ops = [("bar",), W("k", s, 0), ("kp", s, 0), ("shipk", s, 0, 2, 0), *first_q,
               W("v", s, 0), ("qs", s, 1, 0), ("shipv", s, 0, (2,), 0),
               W("k", s, 1), ("bar2",), ("pv", s, 1, 0), ("kp", s, 1), *S(s, 1, 0, 2), ("shipk", s, 1, 2, 0),
               W("wq", 1), ("qp", s, 1, 1), W("v", s, 1), ("qs", s, 1, 1), ("shipv", s, 1, (2,), 0)]
    else:
        def H(which, p, h):
            return ("shiph", which, s, p, h, (0, 3), 0)
        loads = [("k", s, 0, "h0"), ("k", s, 0, "h1"), ("v", s, 0, "h0"), ("wq", 0), ("x", s, 1, 1), ("x", s, 1, 0),
                 ("v", s, 0, "h1")]
        ops = [("bar",), W("k", s, 0, "h0"), H("kT", 0, 0), W("k", s, 0, "h1"), ("kp", s, 0), H("kT", 0, 1),
               W("v", s, 0, "h0"), H("v", 0, 0), *first_q,
               W("v", s, 0, "h1"), H("v", 0, 1), ("bar2",), ("qs", s, 1, 0),
               W("k", s, 1), H("kT", 1, 0), H("kT", 1, 1), ("pv", s, 1, 0), ("kp", s, 1), *S(s, 1, 0, 2),
               W("wq", 1), ("qp", s, 1, 1), W("v", s, 1), ("qs", s, 1, 1), H("v", 1, 0), H("v", 1, 1)]
    loads += [("k", s, 1), ("wq", 1), ("v", s, 1),
              ("k", k, 0), ("x", k, 0), ("k", k, 1), ("v", k, 0), ("v", k, 1), ("x", k, 1), ("wo",)]
    t1 = [((k, 1, h), 0, 2) for h in range(4)]
    ops += [W("k", k, 0), ("pv", s, 1, 1), ("kp", k, 0), *S(s, 1, 1, 2),
            W("x", k, 0), ("qp", k, 0, 0),
            ("rk", k, 0, 1, 2), ("qs", k, 0, 0),
            W("k", k, 1), W("v", k, 0), ("rv", k, 0, 1, 2), ("pv", k, 0, 0), *S(k, 0, 0, 0),
            ("qp", k, 0, 1), ("kp", k, 1),
            ("rk", k, 1, 1, 2), ("qs", k, 0, 1),
            W("v", k, 1), W("x", k, 1), ("rv", k, 1, 1, 2), ("pv", k, 0, 1), ("qp", k, 1, 0), *S(k, 0, 1, 0),
            ("qp", k, 1, 1), ("qs", k, 1, 0), ("qs", k, 1, 1),
            *WR(t1), ("pv", k, 1, 0), ("pv", k, 1, 1), *MS(t1), W("wo")]
    order = ((1, 0), (0, 0), (1, 1), (0, 1), (1, 2), (0, 2), (1, 3), (0, 3)) if dev == 3 else \
            ((1, 0), (1, 1), (0, 0), (1, 2), (0, 1), (1, 3), (0, 2), (0, 3))
    for (t, h) in order:
        ops += F(k, t, h, 2, 0) if t == 1 else F(k, t, h, 0, 2)
    ops += [("pj", k, 0, 0), ("pj", k, 1, 0), ("pj", k, 1, 1), ("pj", k, 0, 1),
            *R(s, 0, 0, 0), ("pj", s, 0, 0), *R(s, 0, 1, 0), ("pj", s, 0, 1), *R(s, 1, 0, 2), ("pj", s, 1, 0),
            ("ws",), *R(s, 1, 1, 2), ("pj", s, 1, 1)]
    return loads, ops


def _chip2():
    def both(h):
        return [((1, 1, h), 1, 3), ((0, 1, h), 3, 1)]

    def heads(*hs):
        return tuple((b, 1, h // 2, h % 2) for h in hs for b in (1, 0))

    def W2(which, p, *rest):
        return [W(which, 1, p, *rest), W(which, 0, p, *rest)]

    def L2(which, p, *rest):
        return [(which, 1, p, *rest), (which, 0, p, *rest)]

    loads = [*L2("k", 0, 0), *L2("v", 0, 0), *L2("k", 1, 0), *L2("v", 1, 0),
             ("wq", 0), ("x", 1, 1), ("x", 0, 1), *L2("k", 0, 1), *L2("v", 0, 1),
             *L2("k", 1, 1, "h0"), ("wq", 1), *L2("k", 1, 1, "h1"), *L2("v", 1, 1), ("wo",)]
    ops = [("bar",)]
    for p in range(2):
        ops += [*W2("k", p, 0), ("kp", 1, p, 0), ("kp", 0, p, 0), ("shipk", 1, p, 1, 3), ("shipk", 0, p, 1, 1),
                *W2("v", p, 0), ("hold",), ("shipv", 1, p, (1,), 3), ("shipv", 0, p, (1,), 1), ("go",)]
    ops += [W("wq", 0), W("x", 1, 1), ("qp", 1, 1, 0), W("x", 0, 1), ("qp", 0, 1, 0),
            *W2("k", 0, 1), ("qsl", heads(0, 1)),
            *W2("v", 0, 1), ("pvh", heads(0)), ("pvh", heads(1)), *WR(both(0)), *MS(both(0)),
            *W2("k", 1, 1, "h0"), W("wq", 1), ("qp", 1, 1, 1), ("qp", 0, 1, 1), ("kpe", 1, 1, 1), ("kpe", 0, 1, 1),
            *WR(both(1)), *MS(both(1)),
            *W2("k", 1, 1, "h1"), *W2("v", 1, 1), ("qsh", heads(2)), ("kp", 1, 1, 1), ("kp", 0, 1, 1),
            *WR(both(2)), ("pvh", heads(2)), ("qsh", heads(3)), *MS(both(2)), ("pvh", heads(3)),
            *WR(both(3)), *MS(both(3)), W("wo")]
    ops += [("fw2", (((1, 1, h), 3, 1, True), ((0, 1, h), 1, 3, True))) for h in range(4)]
    ops += [("pj", 0, 1, 0), ("pj", 1, 1, 0), ("pj", 0, 1, 1), ("pj", 1, 1, 1),
            *R(1, 0, 0, 3), *R(0, 0, 0, 1), ("pj", 1, 0, 0), ("pj", 0, 0, 0),
            *R(1, 0, 1, 3), ("pj", 1, 0, 1), ("ws",), *R(0, 0, 1, 1), ("pj", 0, 0, 1)]
    return loads, ops


def split(key):
    src, dst, ((b, t, h), final) = key
    if t == 1 and ((src == 2 and not final) or (dst == 0 and final)):
        return 4
    if t == 1 and ((dst == 2 and not final and b == {1: 0, 3: 1}[src]) or (src == 2 and final)):
        return 2
    return 1


_PROGRAMS = [_chip0(), _side(1), _chip2(), _side(3)]
_kernel = make_kernel(_PROGRAMS, split)


def pallas_dist_sparse_attn_blocksparse_kvseq_b2_sq256_skv256_hq4_dh64_kernel(
    x: jax.Array,
    Wq: jax.Array,
    K_ext: jax.Array,
    V_ext: jax.Array,
    Wo: jax.Array,
):
    return _kernel(x, Wq, K_ext, V_ext, Wo)
```
